```python
import numpy as np

kernel_name = "dist_rmsnorm_colshard_i_m768_n512"

def setup_inputs():
    x = np.random.randn(768, 2048).astype(np.float32)
    gamma = np.random.randn(2048).astype(np.float32)
    return {"x": x, "gamma": gamma}

def reference(x: np.ndarray, gamma: np.ndarray) -> np.ndarray:
    eps = 1e-5
    rms = np.sqrt(np.mean(x * x, axis=1, keepdims=True) + eps)
    return gamma * x / rms
```

```python
import contextlib
import math

import jax
import jax.numpy as jnp
from jax import lax
from jax.experimental import pallas as pl
from jax.experimental.pallas import tpu as pltpu

N_DEV = 4
EPS = 1e-5
CHUNKS = (256, 256, 128, 64, 64)
NSMEM = 3


def make_kernel(chunks=CHUNKS, nsmem=NSMEM, scopes=False):
    def scope(name):
        return jax.named_scope(name) if scopes else contextlib.nullcontext()

    def kern(x, gamma):
        m, n = x.shape
        n_global = n * N_DEV
        assert sum(chunks) == m
        nc = len(chunks)
        nv = nc - nsmem
        starts = [sum(chunks[:i]) for i in range(nc)]
        mrows = [-(-c // 128) for c in chunks]
        for c in range(nv, nc):
            assert mrows[c] == 1
        smem_base = starts[nv] if nsmem else m
        smem_rows = m - smem_base

        def groups(c):
            for r in range(mrows[c]):
                ng = min(16, (chunks[c] - r * 128) // 8)
                yield r, [(j, starts[c] + r * 128 + j * 8) for j in range(ng)]

        def body(x_hbm, g_hbm, o_ref, xv, gv, sbuf, rbuf, dsm, prep, in_sems, g_sem, send_sems, recv_sems):
            in_copies = []
            for c in range(nc):
                cp = pltpu.make_async_copy(x_hbm.at[pl.ds(starts[c], chunks[c])],
                                           xv.at[pl.ds(starts[c], chunks[c])], in_sems.at[c])
                cp.start()
                in_copies.append(cp)
            gcp = pltpu.make_async_copy(g_hbm, gv, g_sem)
            gcp.start()
            me = lax.axis_index("i")
            barrier = pltpu.get_barrier_semaphore()
            peers = [me ^ 2, me ^ 1, me ^ 3]
            for p in peers:
                pl.semaphore_signal(barrier, inc=1, device_id=(p,), device_id_type=pl.DeviceIdType.MESH)
            lane = lax.broadcasted_iota(jnp.int32, (8, 128), 1)
            sub = lax.broadcasted_iota(jnp.int32, (8, 128), 0)
            diff = lane - sub

            rdmas = []
            for c in range(nc):
                with scope(f"inwait{c}"):
                    in_copies[c].wait()
                for r, gs in groups(c):
                    acc = jnp.zeros((8, 128), jnp.float32)
                    for j, r0 in gs:
                        xb = xv[r0:r0 + 8, :]
                        s = jnp.sum(xb * xb, axis=1, keepdims=True)
                        acc = jnp.where(diff == 8 * j, s, acc)
                    sbuf[c, r:r + 1, :] = jnp.sum(acc, axis=0, keepdims=True)
                if c == 0:
                    with scope("barwait"):
                        pl.semaphore_wait(barrier, N_DEV - 1)
                row = []
                with scope(f"send{c}"):
                    for k, p in enumerate(peers):
                        if k == 0 and c >= nv:
                            dst = dsm.at[pl.ds(c - nv, 1)]
                        else:
                            dst = rbuf.at[c, k, pl.ds(0, mrows[c])]
                        cp = pltpu.make_async_remote_copy(
                            src_ref=sbuf.at[c, pl.ds(0, mrows[c])], dst_ref=dst,
                            send_sem=send_sems.at[c * 3 + k], recv_sem=recv_sems.at[c * 3 + k],
                            device_id=(p,), device_id_type=pl.DeviceIdType.MESH)
                        cp.start()
                        row.append(cp)
                rdmas.append(row)

            gcp.wait()
            gam = gv[...] * math.sqrt(n_global)
            with scope("sendwait"):
                for row in rdmas:
                    for cp in row:
                        cp.wait_send()
            with scope("nbrwait"):
                for c in range(nc):
                    rdmas[c][1].wait_recv()
                    rdmas[c][2].wait_recv()
            part = []
            for c in range(nc):
                mr = mrows[c]
                p = sbuf[c, 0:mr, :] + rbuf[c, 1, 0:mr, :] + rbuf[c, 2, 0:mr, :] + (EPS * n_global)
                part.append(p)
                if c >= nv:
                    pb = jnp.broadcast_to(p, (8, 128))
                    for r, gs in groups(c):
                        for j, r0 in gs:
                            v = jnp.sum(jnp.where(diff == 8 * j, pb, 0.0), axis=1, keepdims=True)
                            prep[r0 - smem_base:r0 - smem_base + 8, :] = jnp.broadcast_to(v, (8, 128))

            for c in range(nc):
                with scope(f"recvwait{c}"):
                    rdmas[c][0].wait_recv()
                if c < nv:
                    mr = mrows[c]
                    inv = lax.rsqrt(part[c] + rbuf[c, 0, 0:mr, :])
                    for r, gs in groups(c):
                        invb = jnp.broadcast_to(inv[r:r + 1, :], (8, 128))
                        for j, r0 in gs:
                            sc = jnp.sum(jnp.where(diff == 8 * j, invb, 0.0), axis=1, keepdims=True)
                            o_ref[r0:r0 + 8, :] = (xv[r0:r0 + 8, :] * gam) * sc
                else:
                    for r, gs in groups(c):
                        for j, r0 in gs:
                            d = jnp.full((8, 128), dsm[c - nv, 8 * j], jnp.float32)
                            for s in range(1, 8):
                                d = jnp.where(sub == s, dsm[c - nv, 8 * j + s], d)
                            inv = lax.rsqrt(prep[r0 - smem_base:r0 - smem_base + 8, :] + d)
                            for q in range(n // 128):
                                o_ref[r0:r0 + 8, q * 128:(q + 1) * 128] = (
                                    xv[r0:r0 + 8, q * 128:(q + 1) * 128] * gam[:, q * 128:(q + 1) * 128]) * inv

        return pl.pallas_call(
            body,
            out_shape=pltpu.VMEM((m, n), x.dtype),
            in_specs=[pl.BlockSpec(memory_space=pl.ANY), pl.BlockSpec(memory_space=pl.ANY)],
            out_specs=pl.BlockSpec(memory_space=pltpu.VMEM),
            scratch_shapes=[
                pltpu.VMEM((m, n), jnp.float32),
                pltpu.VMEM((1, n), jnp.float32),
                pltpu.VMEM((nc, 8, 128), jnp.float32),
                pltpu.VMEM((nc, N_DEV - 1, 8, 128), jnp.float32),
                pltpu.SMEM((max(nsmem, 1), 128), jnp.float32),
                pltpu.VMEM((max(smem_rows, 8), 128), jnp.float32),
                pltpu.SemaphoreType.DMA((nc,)),
                pltpu.SemaphoreType.DMA,
                pltpu.SemaphoreType.DMA((nc * 3,)),
                pltpu.SemaphoreType.DMA((nc * 3,)),
            ],
            compiler_params=pltpu.CompilerParams(collective_id=0, disable_semaphore_checks=True),
        )(x, gamma.reshape(1, n))
    return kern


_KERNEL = make_kernel()


def pallas_dist_rmsnorm_colshard_i_m768_n512_kernel(x, gamma):
    return _KERNEL(x, gamma)
```

```python
import math

import jax
import jax.numpy as jnp
from jax import lax
from jax.experimental import pallas as pl
from jax.experimental.pallas import tpu as pltpu

_N_DEV = 4
_EPS = 1e-5
_LANES = 128
_SUB = 8
_CHUNKS = (256, 256, 128, 80, 48)
_N_SMEM = 3


def _compiler_params():
    try:
        return pltpu.CompilerParams(collective_id=0, disable_semaphore_checks=True)
    except TypeError:
        return pltpu.CompilerParams(collective_id=0)


def pallas_dist_rmsnorm_colshard_i_m768_n512_kernel(
    x: jax.Array,
    gamma: jax.Array,
):
    m, n = x.shape
    n_global = n * _N_DEV
    chunks = _CHUNKS
    assert sum(chunks) == m and n % _LANES == 0
    nc = len(chunks)
    nv = nc - _N_SMEM
    starts = [sum(chunks[:i]) for i in range(nc)]
    mrows = [-(-c // _LANES) for c in chunks]
    assert all(c % _SUB == 0 for c in chunks) and max(mrows) <= _SUB
    assert all(mrows[c] == 1 for c in range(nv, nc))
    smem_base = starts[nv]

    def groups(c):
        for r in range(mrows[c]):
            ng = min(_LANES, chunks[c] - r * _LANES) // _SUB
            yield r, [(j, starts[c] + r * _LANES + j * _SUB) for j in range(ng)]

    def body(x_hbm, g_hbm, o_ref, xv, gv, sbuf, rbuf, dsm, prep,
             in_sems, g_sem, send_sems, recv_sems):
        in_copies = []
        for c in range(nc):
            rows = pl.ds(starts[c], chunks[c])
            cp = pltpu.make_async_copy(x_hbm.at[rows], xv.at[rows], in_sems.at[c])
            cp.start()
            in_copies.append(cp)
        g_copy = pltpu.make_async_copy(g_hbm, gv, g_sem)
        g_copy.start()

        me = lax.axis_index("i")
        peers = [me ^ 2, me ^ 1, me ^ 3]
        barrier = pltpu.get_barrier_semaphore()
        for p in peers:
            pl.semaphore_signal(barrier, inc=1, device_id=(p,),
                                device_id_type=pl.DeviceIdType.MESH)

        lane = lax.broadcasted_iota(jnp.int32, (_SUB, _LANES), 1)
        sub = lax.broadcasted_iota(jnp.int32, (_SUB, _LANES), 0)
        diff = lane - sub

        rdmas = []
        for c in range(nc):
            in_copies[c].wait()
            for r, gs in groups(c):
                acc = jnp.zeros((_SUB, _LANES), jnp.float32)
                for j, r0 in gs:
                    xb = xv[r0:r0 + _SUB, :]
                    s = jnp.sum(xb * xb, axis=1, keepdims=True)
                    acc = jnp.where(diff == _SUB * j, s, acc)
                sbuf[c, r:r + 1, :] = jnp.sum(acc, axis=0, keepdims=True)
            if c == 0:
                pl.semaphore_wait(barrier, _N_DEV - 1)
            row = []
            for k, p in enumerate(peers):
                if k == 0 and c >= nv:
                    dst = dsm.at[pl.ds(c - nv, 1)]
                else:
                    dst = rbuf.at[c, k, pl.ds(0, mrows[c])]
                cp = pltpu.make_async_remote_copy(
                    src_ref=sbuf.at[c, pl.ds(0, mrows[c])],
                    dst_ref=dst,
                    send_sem=send_sems.at[c * 3 + k],
                    recv_sem=recv_sems.at[c * 3 + k],
                    device_id=(p,),
                    device_id_type=pl.DeviceIdType.MESH,
                )
                cp.start()
                row.append(cp)
            rdmas.append(row)

        g_copy.wait()
        gam = gv[...] * math.sqrt(n_global)
        for row in rdmas:
            for cp in row:
                cp.wait_send()

        def partial(c):
            mr = mrows[c]
            return (sbuf[c, 0:mr, :] + rbuf[c, 1, 0:mr, :] + rbuf[c, 2, 0:mr, :]
                    + _EPS * n_global)

        def expand(row_vec, j):
            return jnp.sum(jnp.where(diff == _SUB * j, row_vec, 0.0),
                           axis=1, keepdims=True)

        def finish_vmem(c):
            inv = lax.rsqrt(partial(c) + rbuf[c, 0, 0:mrows[c], :])
            for r, gs in groups(c):
                invb = jnp.broadcast_to(inv[r:r + 1, :], (_SUB, _LANES))
                for j, r0 in gs:
                    o_ref[r0:r0 + _SUB, :] = (xv[r0:r0 + _SUB, :] * gam) * expand(invb, j)

        def finish_smem(c):
            for _, gs in groups(c):
                for j, r0 in gs:
                    d = jnp.full((_SUB, _LANES), dsm[c - nv, _SUB * j], jnp.float32)
                    for s in range(1, _SUB):
                        d = jnp.where(sub == s, dsm[c - nv, _SUB * j + s], d)
                    p0 = r0 - smem_base
                    inv = lax.rsqrt(prep[p0:p0 + _SUB, :] + d)
                    for q in range(n // _LANES):
                        cols = slice(q * _LANES, (q + 1) * _LANES)
                        o_ref[r0:r0 + _SUB, cols] = (xv[r0:r0 + _SUB, cols] * gam[:, cols]) * inv

        for k in (1, 2, 0):
            rdmas[0][k].wait_recv()
        finish_vmem(0)

        for c in range(1, nc):
            rdmas[c][1].wait_recv()
            rdmas[c][2].wait_recv()
        for c in range(nv, nc):
            pb = jnp.broadcast_to(partial(c), (_SUB, _LANES))
            for _, gs in groups(c):
                for j, r0 in gs:
                    p0 = r0 - smem_base
                    prep[p0:p0 + _SUB, :] = jnp.broadcast_to(expand(pb, j), (_SUB, _LANES))

        for c in range(1, nc):
            rdmas[c][0].wait_recv()
            if c < nv:
                finish_vmem(c)
            else:
                finish_smem(c)

    return pl.pallas_call(
        body,
        out_shape=jax.ShapeDtypeStruct((m, n), x.dtype),
        in_specs=[
            pl.BlockSpec(memory_space=pl.ANY),
            pl.BlockSpec(memory_space=pl.ANY),
        ],
        out_specs=pl.BlockSpec(memory_space=pltpu.VMEM),
        scratch_shapes=[
            pltpu.VMEM((m, n), jnp.float32),
            pltpu.VMEM((1, n), jnp.float32),
            pltpu.VMEM((nc, _SUB, _LANES), jnp.float32),
            pltpu.VMEM((nc, _N_DEV - 1, _SUB, _LANES), jnp.float32),
            pltpu.SMEM((_N_SMEM, _LANES), jnp.float32),
            pltpu.VMEM((m - smem_base, _LANES), jnp.float32),
            pltpu.SemaphoreType.DMA((nc,)),
            pltpu.SemaphoreType.DMA,
            pltpu.SemaphoreType.DMA((nc * 3,)),
            pltpu.SemaphoreType.DMA((nc * 3,)),
        ],
        compiler_params=_compiler_params(),
    )(x, gamma.reshape(1, n))
```
